```python
import numpy as np

kernel_name = "dist_ar_xy_y_m1024_n512"

def setup_inputs():
    return {"x": np.random.randn(2048, 512).astype(np.float32)}

def reference(x: np.ndarray) -> np.ndarray:
    return x.reshape(2, 1024, 512).sum(axis=0)
```

```python
import jax
import jax.numpy as jnp
from jax import lax
from jax.experimental import pallas as pl
from jax.experimental.pallas import tpu as pltpu

M, N = 1024, 512
ROWS, LANES = 16, 128
TILES_PER_BLOCK = N // LANES
Y_TILES = 138
X_TILES = M // ROWS * TILES_PER_BLOCK - Y_TILES
Y_BLOCKS = -(-Y_TILES // TILES_PER_BLOCK)
LOADS = (1, 1, 2, 4)
AHEAD = sum(LOADS)
MESH = pl.DeviceIdType.MESH


def _body(x_hbm, out, own, send_buf, recv_buf, load_sems, y_send, y_recv,
          x_send, x_recv, x_ready):
    mx, my = lax.axis_index("x"), lax.axis_index("y")
    y_peer, x_peer = (mx, 1 - my), (1 - mx, my)

    barrier = pltpu.get_barrier_semaphore()
    pl.semaphore_signal(barrier, 1, device_id=y_peer, device_id_type=MESH)

    @pl.when(mx == 0)
    def _():
        pl.semaphore_signal(barrier, 1, device_id=x_peer, device_id_type=MESH)

    step = 1 - 2 * mx

    def rows(b, n=1):
        start = mx * (M - n * ROWS) + step * (b * ROWS)
        return pl.ds(pl.multiple_of(start, ROWS), n * ROWS)

    def tile(b, j):
        start = mx * (N - LANES) + step * (j * LANES)
        return rows(b), pl.ds(pl.multiple_of(start, LANES), LANES)

    spans, b0 = [], 0
    for n in (*LOADS, Y_BLOCKS - AHEAD):
        spans.append((b0, n))
        b0 += n
    loads = [
        pltpu.make_async_copy(x_hbm.at[rows(b, n)], own.at[rows(b, n)],
                              load_sems.at[i])
        for i, (b, n) in enumerate(spans)
    ]
    for load in loads:
        load.start()

    pl.semaphore_wait(barrier, 1 + mx)

    @pl.when(mx == 1)
    def _():
        pl.semaphore_signal(x_ready, 1, device_id=x_peer, device_id_type=MESH)

    def y_copy(b, j):
        return pltpu.make_async_remote_copy(
            send_buf.at[tile(b, j)], recv_buf.at[tile(b, j)], y_send,
            y_recv.at[b * TILES_PER_BLOCK + j],
            device_id=y_peer, device_id_type=MESH)

    def send(b, j):
        send_buf[tile(b, j)] = own[tile(b, j)].astype(jnp.bfloat16)
        y_copy(b, j).start()

    def reduce(b, j, forward):
        y_copy(b, j).wait_recv()
        t = tile(b, j)
        out[t] = (own[t] + recv_buf[t].astype(jnp.float32)).astype(out.dtype)
        if forward:
            pltpu.make_async_remote_copy(
                out.at[t], out.at[t], x_send, x_recv,
                device_id=x_peer, device_id_type=MESH).start()

    for load, (b0, n) in zip(loads[:-1], spans):
        load.wait()
        for b in range(b0, b0 + n):
            for j in range(TILES_PER_BLOCK):
                send(b, j)

    @pl.when(mx == 0)
    def _():
        pl.semaphore_wait(x_ready, 1)

    for j in range(TILES_PER_BLOCK):
        reduce(0, j, True)
    loads[-1].wait()
    for j in range(TILES_PER_BLOCK):
        send(AHEAD, j)

    def plan(b):
        ts = range(b * TILES_PER_BLOCK, (b + 1) * TILES_PER_BLOCK)
        return tuple((t < Y_TILES, t < X_TILES,
                      t + AHEAD * TILES_PER_BLOCK < Y_TILES) for t in ts)

    def run_block(b, what):
        for j, (receives, forwards, sends) in enumerate(what):
            if receives:
                reduce(b, j, forwards)
            if sends:
                send(b + AHEAD, j)

    b = 1
    while b < Y_BLOCKS:
        end = b + 1
        while end < Y_BLOCKS and plan(end) == plan(b):
            end += 1
        if end == b + 1:
            run_block(b, plan(b))
        else:
            lax.fori_loop(b, end, lambda i, _, p=plan(b): run_block(i, p), None)
        b = end

    def all_of(n_tiles, sem):
        view = recv_buf.at[pl.ds(0, n_tiles // 2 * ROWS), pl.ds(0, 2 * LANES)]
        return pltpu.make_async_remote_copy(
            view, view, sem, sem, device_id=x_peer, device_id_type=MESH)

    view = send_buf.at[pl.ds(0, Y_TILES // 3 * ROWS), pl.ds(0, 3 * LANES)]
    pltpu.make_async_remote_copy(
        view, view, y_send, y_send,
        device_id=y_peer, device_id_type=MESH).wait_send()
    all_of(X_TILES, x_send).wait_send()
    all_of(X_TILES, x_recv).wait_recv()


def pallas_dist_ar_xy_y_m1024_n512_kernel(x: jax.Array):
    assert Y_TILES % 3 == 0 and X_TILES % 2 == 0
    return pl.pallas_call(
        _body,
        out_shape=jax.ShapeDtypeStruct((M, N), jnp.bfloat16),
        in_specs=[pl.BlockSpec(memory_space=pl.ANY)],
        out_specs=pl.BlockSpec(memory_space=pltpu.VMEM),
        scratch_shapes=[
            pltpu.VMEM((M, N), jnp.float32),
            pltpu.VMEM((M, N), jnp.bfloat16),
            pltpu.VMEM((M, N), jnp.bfloat16),
            pltpu.SemaphoreType.DMA((len(LOADS) + 1,)),
            pltpu.SemaphoreType.DMA,
            pltpu.SemaphoreType.DMA((Y_TILES,)),
            pltpu.SemaphoreType.DMA,
            pltpu.SemaphoreType.DMA,
            pltpu.SemaphoreType.REGULAR,
        ],
        compiler_params=pltpu.CompilerParams(
            collective_id=0,
            disable_bounds_checks=True,
            disable_semaphore_checks=True,
        ),
    )(x)
```

```python
import jax
import jax.numpy as jnp
from jax import lax
from jax.experimental import pallas as pl
from jax.experimental.pallas import tpu as pltpu

M, N = 1024, 512
LANES = 128
VREG = (8, LANES)

HEAD, ROWS = 8, 16
TILES = N // LANES
BLOCKS = (M - 2 * HEAD) // ROWS
Y_BLOCKS = 35
X_BLOCKS = BLOCKS - Y_BLOCKS

QUEUE = 4
GROUP, CODE_SLOTS, BYTE_SLOTS = 4, 3, 2
ESCAPE = 7
ENTRY_BITS = 5
FIRST_CODED = 23
HEADER_BITS = 9
OVERFLOW = 256

FIRST_LOADS = (1, 3, 8)
EARLY_X_BLOCKS = 16

MESH = pl.DeviceIdType.MESH
srl = lax.shift_right_logical


def _code_slot(block):
    return QUEUE + (CODE_SLOTS + GROUP * BYTE_SLOTS) * (block // GROUP)


def _byte_slot(block):
    return _code_slot(block) + CODE_SLOTS + BYTE_SLOTS * (block % GROUP)


def _end_slot(block):
    return _byte_slot(block) + BYTE_SLOTS


Y_SLOTS = _end_slot(Y_BLOCKS - 1)
X_SLOTS = _end_slot(X_BLOCKS - 1)
X_PARTS = [(0, _end_slot(EARLY_X_BLOCKS - 1))] + [
    (_end_slot(b - 1), _end_slot(b)) for b in range(EARLY_X_BLOCKS, X_BLOCKS)
]


def _both(v):
    v *= 0x10001
    return v - (1 << 32) if v >= 1 << 31 else v


def _shift_left(words, n):
    carry = 31 - n
    return [words[0] << n] + [
        (hi << n) | srl(srl(lo, 1), carry) for lo, hi in zip(words, words[1:])
    ]


class _Encoder:
    def __init__(self, stream):
        self.stream = stream
        zero = jnp.zeros(VREG, jnp.int32)
        self.queue = [zero] * QUEUE
        self.queue_bits = zero
        self.outside = zero

    def place_window(self, tiles):
        logs = [(srl(w, 16) & 0x7FFF) + (w & 0x7FFF) for w in tiles]
        total = ((logs[0] + logs[1]) + (logs[2] + logs[3])).astype(jnp.float32)
        total = jnp.sum(total, axis=0, keepdims=True)
        total = jnp.sum(total, axis=1, keepdims=True)
        mean = total * (1.0 / (128 * ROWS * N))
        base = jnp.clip(mean + (3.26 - ESCAPE - FIRST_CODED), 0.0, 224.0)
        self.base = jnp.broadcast_to(base, VREG).astype(jnp.int32)
        self.offset = _both(256) - (self.base | (self.base << 16))

    def put_bytes(self, block, tiles):
        slots = [_byte_slot(block) + k for k in range(BYTE_SLOTS)]
        for slot, a, b in zip(slots, tiles[0::2], tiles[1::2]):
            self.stream[slot] = (
                (a & _both(0x807F))
                | ((b << 7) & _both(0x3F80))
                | (srl(b, 1) & _both(0x4000))
            )
        return slots

    def put_exponents(self, block, tiles):
        if block % GROUP == 0:
            self.codes = [0] * CODE_SLOTS
        for j, w in enumerate(tiles):
            entry = (srl(w, 7) & _both(255)) + self.offset
            self.outside |= entry ^ _both(256)
            code = (entry + _both(32 - FIRST_CODED)) & _both(31)
            escaped = (code + _both(32 - ESCAPE)) & _both(32)
            escaped = escaped - srl(escaped, 5)
            code = (code | escaped) & _both(ESCAPE)

            t = TILES * (block % GROUP) + j
            if t < 15:
                self.codes[t // 5] |= code << (3 * (t % 5))
            else:
                for k in range(CODE_SLOTS):
                    self.codes[k] |= (code << (15 - k)) & _both(0x8000)

            entry &= escaped
            bits = escaped & _both(ENTRY_BITS)
            if j % 2 == 0:
                new, new_bits = entry & 31, bits
            else:
                new, new_bits = (new << (bits & 31)) | (entry & 31), new_bits + bits
            new = (new << srl(bits, 16)) | srl(entry, 16)
            if j % 2 == 1:
                new_bits = (new_bits & 31) + srl(new_bits, 16)
                self.queue = _shift_left(self.queue, new_bits)
                self.queue[0] |= new
                self.queue_bits += new_bits
        if block % GROUP < GROUP - 1 and block < Y_BLOCKS - 1:
            return []
        slots = [_code_slot(block) + k for k in range(CODE_SLOTS)]
        for slot, codes in zip(slots, self.codes):
            self.stream[slot] = codes
        return slots

    def put_queue(self):
        overflow = (self.queue_bits > 32 * QUEUE - HEADER_BITS) | (
            (self.outside & _both(0x1E0)) != 0
        )
        gap = jnp.maximum(32 * QUEUE - self.queue_bits, 0)
        queue = self.queue
        for n in (2, 1):
            move = (gap & (32 * n)) != 0
            queue = [
                jnp.where(move, queue[i - n] if i >= n else 0, queue[i])
                for i in range(QUEUE)
            ]
        queue = _shift_left(queue, gap & 31)
        header = self.base | jnp.where(overflow, OVERFLOW, 0)
        queue[0] = (queue[0] & -(1 << HEADER_BITS)) | header
        for slot in range(QUEUE):
            self.stream[slot] = queue[slot]
        return list(range(QUEUE))


class _Decoder:
    def __init__(self, stream):
        self.stream = stream
        self.queue = [stream[slot] for slot in range(QUEUE)]
        base = self.queue[0] & 255
        self.base = base | (base << 16)

    def exponents(self, block):
        slot = _code_slot(block)
        tiles = []
        for j in range(TILES):
            t = TILES * (block % GROUP) + j
            if t < 15:
                code = srl(self.stream[slot + t // 5], 3 * (t % 5)) & _both(7)
            else:
                code = 0
                for k in range(CODE_SLOTS):
                    code |= srl(self.stream[slot + k] & _both(0x8000), 15 - k)
            entry = code + _both(FIRST_CODED)
            if j % 2 == 0:
                top, used = self.queue[-1], 0
            halves = []
            for half in (entry & 31, srl(entry, 16)):
                escaped = half == FIRST_CODED + ESCAPE
                halves.append(jnp.where(escaped, srl(top, 32 - ENTRY_BITS), half))
                top = jnp.where(escaped, top << ENTRY_BITS, top)
                used = jnp.where(escaped, used + ENTRY_BITS, used)
            if j % 2 == 1:
                self.queue = _shift_left(self.queue, used)
            tiles.append(((halves[0] | (halves[1] << 16)) + self.base) << 7)
        return tiles


def _body(x_hbm, out, own, tx, from_y, from_x, head, exp_tx, exp_from_y,
          exp_from_x, load_sems, head_send, head_recv, y_send, y_recv, x_send,
          x_recv, sum_send, sum_recv, exp_send, exp_recv, x_ready):
    mx, my = lax.axis_index("x"), lax.axis_index("y")
    y_peer, x_peer = (mx, 1 - my), (1 - mx, my)

    def span(start, size):
        first = mx * (M - size) + (1 - 2 * mx) * start
        return pl.ds(pl.multiple_of(first, HEAD), size)

    def rows(block, n=1):
        return span(HEAD + block * ROWS, n * ROWS)

    def relayed_rows(block):
        return rows(BLOCKS - 1 - block)

    def remote(src, dst, send_sem, recv_sem, peer):
        return pltpu.make_async_remote_copy(
            src, dst, send_sem, recv_sem, device_id=peer, device_id_type=MESH)

    spans, start = [], 0
    for n in (*FIRST_LOADS, Y_BLOCKS - sum(FIRST_LOADS), X_BLOCKS):
        spans.append(rows(start, n))
        start += n
    spans.append(span(0, HEAD))
    *first_loads, y_load, x_load, head_load = [
        pltpu.make_async_copy(x_hbm.at[s], own.at[s], load_sems.at[i])
        for i, s in enumerate(spans)
    ]

    first_loads[0].start()
    barrier = pltpu.get_barrier_semaphore()
    pl.semaphore_signal(barrier, 1, device_id=y_peer, device_id_type=MESH)

    @pl.when(mx == 0)
    def _():
        pl.semaphore_signal(barrier, 1, device_id=x_peer, device_id_type=MESH)

    for load in (*first_loads[1:], y_load):
        load.start()
    pl.semaphore_wait(barrier, 1 + mx)

    halves = [pl.ds(j * N // 2, N // 2) for j in range(2)]
    head_copies = [
        remote(x_hbm.at[span(0, HEAD), cols], head.at[:, cols],
               head_send.at[j], head_recv.at[j], y_peer)
        for j, cols in enumerate(halves)
    ]
    for copy in (*head_copies, head_load, x_load):
        copy.start()

    @pl.when(mx == 1)
    def _():
        pl.semaphore_signal(x_ready, 1, device_id=x_peer, device_id_type=MESH)

    def bf16_pairs(block):
        w = pltpu.bitcast(own[rows(block), :].astype(jnp.bfloat16), jnp.int32)
        return [w[:, j * LANES:(j + 1) * LANES] for j in range(TILES)]

    def add(stream, block, where, exponents):
        tiles = []
        for k in range(BYTE_SLOTS):
            b = stream[_byte_slot(block) + k]
            tiles.append(b & _both(0x807F))
            tiles.append((srl(b, 7) & _both(0x7F)) | ((b << 1) & _both(0x8000)))
        w = jnp.concatenate([t | e for t, e in zip(tiles, exponents)], axis=1)
        other = pltpu.bitcast(w, jnp.bfloat16).astype(jnp.float32)
        out[where, :] = (own[where, :] + other).astype(out.dtype)

    def y_copy(slot):
        return remote(tx.at[slot], from_y.at[slot], y_send, y_recv.at[slot], y_peer)

    sent, arrived = [], set()

    def send(slots):
        for slot in slots:
            y_copy(slot).start()
            sent.append(slot)

    def receive(slot):
        y_copy(slot).wait_recv()
        arrived.add(slot)

    def missing(block):
        return [s for s in range(_code_slot(block), _end_slot(block))
                if s not in arrived]

    encoder = _Encoder(tx)
    encoded = 0
    for load, n in zip(first_loads, FIRST_LOADS):
        load.wait()
        for block in range(encoded, encoded + n):
            tiles = bf16_pairs(block)
            send(encoder.put_bytes(block, tiles))
            if block == 0:
                encoder.place_window(tiles)
                first_tiles = tiles
                continue
            if block == 1:
                send(encoder.put_exponents(0, first_tiles))
            send(encoder.put_exponents(block, tiles))
        encoded += n

    @pl.when(mx == 0)
    def _():
        pl.semaphore_wait(x_ready, 1)

    head_load.wait()
    sum_copies = []
    for j, cols in enumerate(halves):
        at = (span(0, HEAD), cols)
        head_copies[j].wait_recv()
        out[at] = (own[at] + head[:, cols]).astype(out.dtype)
        sum_copies.append(
            remote(out.at[at], out.at[at], sum_send.at[j], sum_recv, x_peer))
        sum_copies[-1].start()

    y_load.wait()
    ready, held = [], []
    y_decoder, y_added = None, 0
    for i in range(X_SLOTS):
        slot = sent[i]
        receive(slot)
        part = next(p for p, (lo, hi) in enumerate(X_PARTS) if lo <= slot < hi)
        remote(from_y.at[slot], from_x.at[slot], x_send, x_recv.at[part],
               x_peer).start()
        if ready:
            send([ready.pop(0)])
        if encoded < Y_BLOCKS:
            tiles = bf16_pairs(encoded)
            held += encoder.put_bytes(encoded, tiles)
            codes = encoder.put_exponents(encoded, tiles)
            if codes:
                ready, held = ready + codes + held, []
            encoded += 1
        elif 0 not in sent:
            send(encoder.put_queue())
        if y_decoder is None and arrived.issuperset(range(QUEUE)):
            y_decoder = _Decoder(from_y)
        if y_decoder is not None and not missing(y_added):
            add(from_y, y_added, rows(y_added), y_decoder.exponents(y_added))
            y_added += 1
    send(ready)

    def receive_part(part):
        lo, hi = X_PARTS[part]
        remote(from_y.at[lo:hi], from_x.at[lo:hi], x_send, x_recv.at[part],
               x_peer).wait_recv()

    def overflowed(stream):
        return stream[0] & OVERFLOW

    x_load.wait()
    receive_part(0)
    x_decoder = _Decoder(from_x)
    any_overflow = jnp.max(
        overflowed(tx) | overflowed(from_y) | overflowed(from_x)) > 0
    while not missing(y_added):
        add(from_y, y_added, rows(y_added), y_decoder.exponents(y_added))
        y_added += 1
    for block in range(X_BLOCKS - 1):
        if X_BLOCKS - block <= Y_BLOCKS - y_added:
            for slot in missing(y_added):
                receive(slot)
            add(from_y, y_added, rows(y_added), y_decoder.exponents(y_added))
            y_added += 1
        if block >= EARLY_X_BLOCKS:
            receive_part(block - EARLY_X_BLOCKS + 1)
        add(from_x, block, relayed_rows(block), x_decoder.exponents(block))

    assert y_added == Y_BLOCKS - 1
    last_y = y_decoder.exponents(Y_BLOCKS - 1)
    last_x = x_decoder.exponents(X_BLOCKS - 1)
    for copy in (*head_copies, *sum_copies):
        copy.wait_send()
    far_head = out.at[span(M - HEAD, HEAD)]
    remote(far_head, far_head, sum_recv, sum_recv, x_peer).wait_recv()
    remote(from_y.at[:X_SLOTS], from_x, x_send, x_send, x_peer).wait_send()
    remote(tx, from_y, y_send, y_send, y_peer).wait_send()
    for slot in missing(y_added):
        receive(slot)
    add(from_y, Y_BLOCKS - 1, rows(Y_BLOCKS - 1), last_y)
    receive_part(len(X_PARTS) - 1)
    add(from_x, X_BLOCKS - 1, relayed_rows(X_BLOCKS - 1), last_x)
    assert sorted(sent) == sorted(arrived) == list(range(Y_SLOTS))

    @pl.when(any_overflow)
    def _():
        y_exp = remote(exp_tx, exp_from_y, exp_send.at[0], exp_recv.at[0], y_peer)
        x_exp = remote(exp_from_y.at[:2 * X_BLOCKS], exp_from_x,
                       exp_send.at[1], exp_recv.at[1], x_peer)

        def redo(stream, full, n_blocks, where):
            @pl.loop(0, n_blocks)
            def _(block):
                a, b = full[2 * block], full[2 * block + 1]
                shifted = (a << 7, srl(a, 1), b << 7, srl(b, 1))
                add(stream, block, where(block),
                    [e & _both(0x7F80) for e in shifted])

        mine = jnp.max(overflowed(tx)) > 0

        @pl.when(mine)
        def _():
            @pl.loop(0, Y_BLOCKS)
            def _(block):
                tiles = bf16_pairs(block)
                for k in range(2):
                    a, b = tiles[2 * k], tiles[2 * k + 1]
                    exp_tx[2 * block + k] = (
                        (srl(a, 7) & _both(0xFF)) | ((b << 1) & _both(0xFF00)))

            y_exp.start()

        @pl.when(jnp.max(overflowed(from_y)) > 0)
        def _():
            y_exp.wait_recv()
            x_exp.start()
            redo(from_y, exp_from_y, Y_BLOCKS, rows)
            x_exp.wait_send()

        @pl.when(jnp.max(overflowed(from_x)) > 0)
        def _():
            x_exp.wait_recv()
            redo(from_x, exp_from_x, X_BLOCKS, relayed_rows)

        @pl.when(mine)
        def _():
            y_exp.wait_send()


def pallas_dist_ar_xy_y_m1024_n512_kernel(x: jax.Array):
    dma = pltpu.SemaphoreType.DMA
    return pl.pallas_call(
        _body,
        out_shape=jax.ShapeDtypeStruct((M, N), jnp.bfloat16),
        in_specs=[pl.BlockSpec(memory_space=pl.ANY)],
        out_specs=pl.BlockSpec(memory_space=pltpu.VMEM),
        scratch_shapes=[
            pltpu.VMEM((M, N), jnp.float32),
            pltpu.VMEM((Y_SLOTS, *VREG), jnp.int32),
            pltpu.VMEM((Y_SLOTS, *VREG), jnp.int32),
            pltpu.VMEM((X_SLOTS, *VREG), jnp.int32),
            pltpu.VMEM((HEAD, N), jnp.float32),
            pltpu.VMEM((2 * Y_BLOCKS, *VREG), jnp.int32),
            pltpu.VMEM((2 * Y_BLOCKS, *VREG), jnp.int32),
            pltpu.VMEM((2 * X_BLOCKS, *VREG), jnp.int32),
            dma((len(FIRST_LOADS) + 3,)),
            dma((2,)),
            dma((2,)),
            dma,
            dma((Y_SLOTS,)),
            dma,
            dma((len(X_PARTS),)),
            dma((2,)),
            dma,
            dma((2,)),
            dma((2,)),
            pltpu.SemaphoreType.REGULAR,
        ],
        compiler_params=pltpu.CompilerParams(
            collective_id=0,
            disable_bounds_checks=True,
            disable_semaphore_checks=True,
        ),
    )(x)
```

```python
import jax
import jax.numpy as jnp
from jax import lax
from jax.experimental import pallas as pl
from jax.experimental.pallas import tpu as pltpu

M, N = 1024, 512
LANES = 128
VREG = (8, LANES)

HEAD, ROWS = 8, 16
TILES = N // LANES
BLOCKS = (M - 2 * HEAD) // ROWS
Y_BLOCKS = 35
X_BLOCKS = BLOCKS - Y_BLOCKS

QUEUE_SLOTS, CODE_SLOTS, BYTE_SLOTS = 2, 3, 2
GROUP = 4
ESCAPE = 7
ABOVE = 6
HEADER_BITS = 2
UNNUDGED_BLOCKS = 2

FIRST_LOADS = (1, 1, 2, 4, 4)
EARLY_X_BLOCKS = 16
REDO_BLOCKS = 7

MESH = pl.DeviceIdType.MESH
srl = lax.shift_right_logical


def _code_slot(block):
    return QUEUE_SLOTS + (CODE_SLOTS + GROUP * BYTE_SLOTS) * (block // GROUP)


def _byte_slot(block):
    return _code_slot(block) + CODE_SLOTS + BYTE_SLOTS * (block % GROUP)


def _end_slot(block):
    return _byte_slot(block) + BYTE_SLOTS


Y_SLOTS = _end_slot(Y_BLOCKS - 1)
X_SLOTS = _end_slot(X_BLOCKS - 1)
X_PARTS = [(0, _end_slot(EARLY_X_BLOCKS - 1))] + [
    (_end_slot(b - 1), _end_slot(b)) for b in range(EARLY_X_BLOCKS, X_BLOCKS)
]


def _both(v):
    v *= 0x10001
    return v - (1 << 32) if v >= 1 << 31 else v


def _shift_left(low, high, n):
    return low << n, (high << n) | srl(srl(low, 1), 31 - n)


def _header_shift():
    return HEADER_BITS * lax.broadcasted_iota(jnp.int32, VREG, 0)


class _Window:
    def __init__(self, position):
        self.top = srl(position, 7)
        nudge = ~position & 127
        self.nudges = nudge | (nudge << 16)

    def nudge(self, block):
        return jnp.where(block < UNNUDGED_BLOCKS, 0, self.nudges)


class _Encoder:
    def __init__(self, stream):
        self.stream = stream
        zero = jnp.zeros(VREG, jnp.int32)
        self.low = self.high = self.queue_bits = self.longest_move = zero

    def place_window(self, tiles):
        logs = [(srl(w, 16) & 0x7FFF) + (w & 0x7FFF) for w in tiles]
        total = ((logs[0] + logs[1]) + (logs[2] + logs[3])).astype(jnp.float32)
        total = jnp.sum(total, axis=0, keepdims=True)
        total = jnp.sum(total, axis=1, keepdims=True)
        position = jnp.minimum(total * (1 / (ROWS * N)) + 2.75 * 128, 32767.0)
        self.position = jnp.broadcast_to(position, VREG).astype(jnp.int32)
        self.window = _Window(self.position)
        self.tops = _both(256) + (self.window.top | (self.window.top << 16))

    def put_bytes(self, block, tiles):
        slots = [_byte_slot(block) + k for k in range(BYTE_SLOTS)]
        for slot, a, b in zip(slots, tiles[0::2], tiles[1::2]):
            self.stream[slot] = (
                (a & _both(0x807F))
                | ((b << 7) & _both(0x3F80))
                | (srl(b, 1) & _both(0x4000))
            )
        return slots

    def put_exponents(self, block, tiles):
        if block % GROUP == 0:
            self.codes = [0] * CODE_SLOTS
        for j, w in enumerate(tiles):
            depths = (self.tops - (srl(w, 7) & _both(255))) & _both(255)
            escaped = (depths + _both(256 - ESCAPE)) & _both(256)
            code = (depths | (escaped - srl(escaped, 8))) & _both(ESCAPE)

            t = TILES * (block % GROUP) + j
            if t < 15:
                self.codes[t // 5] |= code << (3 * (t % 5))
            else:
                for k in range(CODE_SLOTS):
                    self.codes[k] |= (code << (15 - k)) & _both(0x8000)

            if j % 2 == 0:
                new, new_bits = 0, 0
            for depth in (depths & 255, srl(depths, 16)):
                bits = jnp.clip(depth - (ESCAPE - 1), 0, 30)
                bits = jnp.where(bits >= ABOVE, bits + 1, bits)
                bits = jnp.where(depth == 255, ABOVE, bits)
                new = (new << bits) | jnp.minimum(bits, 1)
                new_bits += bits
            if j % 2 == 1:
                low, self.high = _shift_left(self.low, self.high, new_bits & 31)
                self.low = low | new
                self.queue_bits += new_bits
                self.longest_move = jnp.maximum(self.longest_move, new_bits)
        if block % GROUP < GROUP - 1 and block < Y_BLOCKS - 1:
            return []
        slots = [_code_slot(block) + k for k in range(CODE_SLOTS)]
        for slot, codes in zip(slots, self.codes):
            self.stream[slot] = codes
        return slots

    def put_queue(self):
        gap = 64 - self.queue_bits
        low, high = _shift_left(
            jnp.where(gap >= 32, 0, self.low),
            jnp.where(gap >= 32, self.low, self.high),
            gap & 31)
        header = srl(self.position, _header_shift()) & ((1 << HEADER_BITS) - 1)
        overflow = (gap < HEADER_BITS) | (self.longest_move >= 31)
        self.stream[0] = (low & -(1 << HEADER_BITS)) | header
        self.stream[1] = jnp.where(overflow, -1, high)
        return list(range(QUEUE_SLOTS))


def _overflowed(stream):
    return jnp.where(stream[1] == -1, 1, 0)


class _Decoder:
    def __init__(self, stream):
        self.stream = stream
        self.low, self.high = stream[0], stream[1]
        header = (self.low & ((1 << HEADER_BITS) - 1)) << _header_shift()
        position = jnp.sum(header, axis=0, keepdims=True)
        self.window = _Window(jnp.broadcast_to(position, VREG))

    def exponents(self, block):
        slot = _code_slot(block)
        tiles = []
        for j in range(TILES):
            t = TILES * (block % GROUP) + j
            if t < 15:
                codes = srl(self.stream[slot + t // 5], 3 * (t % 5))
            else:
                codes = 0
                for k in range(CODE_SLOTS):
                    codes |= srl(self.stream[slot + k] & _both(0x8000), 15 - k)
            if j % 2 == 0:
                front, used = self.high | 1, 0
            halves = []
            for code in (codes & ESCAPE, srl(codes, 16) & ESCAPE):
                escaped = code == ESCAPE
                zeros = lax.clz(front)
                front = jnp.where(escaped, (front << 1) << zeros, front)
                used = jnp.where(escaped, (used + 1) + zeros, used)
                depth = zeros + jnp.where(zeros >= ABOVE, ESCAPE - 1, ESCAPE)
                depth = jnp.where(zeros == ABOVE - 1, -1, depth)
                depth = jnp.where(escaped, depth, code)
                halves.append((self.window.top - depth) & 255)
            if j % 2 == 1:
                self.low, self.high = _shift_left(self.low, self.high, used)
            tiles.append((halves[0] << 7) | (halves[1] << 23))
        return tiles


def _body(x_hbm, out, own, tx, from_y, from_x, head, exp_tx, exp_from_y,
          exp_from_x, load_sems, head_send, head_recv, y_send, y_recv, x_send,
          x_recv, sum_send, sum_recv, exp_y_send, exp_y_recv, exp_x_send,
          exp_x_recv, x_ready):
    mx, my = lax.axis_index("x"), lax.axis_index("y")
    y_peer, x_peer = (mx, 1 - my), (1 - mx, my)

    def span(start, size):
        first = mx * (M - size) + (1 - 2 * mx) * start
        return pl.ds(pl.multiple_of(first, HEAD), size)

    def rows(block, n=1):
        return span(HEAD + block * ROWS, n * ROWS)

    def relayed_rows(block):
        return rows(BLOCKS - 1 - block)

    def remote(src, dst, send_sem, recv_sem, peer):
        return pltpu.make_async_remote_copy(
            src, dst, send_sem, recv_sem, device_id=peer, device_id_type=MESH)

    def wait_until_filled(buf, recv_sem):
        pltpu.make_async_copy(buf, buf, recv_sem).wait()

    spans, start = [], 0
    for n in (*FIRST_LOADS, Y_BLOCKS - sum(FIRST_LOADS), X_BLOCKS):
        spans.append(rows(start, n))
        start += n
    spans.append(span(0, HEAD))
    *first_loads, y_load, x_load, head_load = [
        pltpu.make_async_copy(x_hbm.at[s], own.at[s], load_sems.at[i])
        for i, s in enumerate(spans)
    ]

    barrier = pltpu.get_barrier_semaphore()
    pl.semaphore_signal(barrier, 1, device_id=y_peer, device_id_type=MESH)
    first_loads[0].start()

    @pl.when(mx == 0)
    def _():
        pl.semaphore_signal(barrier, 1, device_id=x_peer, device_id_type=MESH)

    for load in (*first_loads[1:], y_load):
        load.start()
    pl.semaphore_wait(barrier, 1 + mx)

    halves = [pl.ds(j * N // 2, N // 2) for j in range(2)]
    head_copies = [
        remote(x_hbm.at[span(0, HEAD), cols], head.at[:, cols],
               head_send.at[j], head_recv.at[j], y_peer)
        for j, cols in enumerate(halves)
    ]
    for copy in (*head_copies, head_load, x_load):
        copy.start()

    @pl.when(mx == 1)
    def _():
        pl.semaphore_signal(x_ready, 1, device_id=x_peer, device_id_type=MESH)

    def pairs(block, nudge):
        w = pltpu.bitcast(own[rows(block), :].astype(jnp.bfloat16), jnp.int32)
        return [w[:, j * LANES:(j + 1) * LANES] + nudge for j in range(TILES)]

    def add(decoder, block, where, exponents=None):
        exponents = exponents or decoder.exponents(block)
        nudge = decoder.window.nudge(block)
        tiles = []
        for k in range(BYTE_SLOTS):
            b = decoder.stream[_byte_slot(block) + k]
            tiles.append(b & _both(0x807F))
            tiles.append((srl(b, 7) & _both(0x7F)) | ((b << 1) & _both(0x8000)))
        w = jnp.concatenate(
            [(t | e) - nudge for t, e in zip(tiles, exponents)], axis=1)
        other = pltpu.bitcast(w, jnp.bfloat16).astype(jnp.float32)
        out[where, :] = (own[where, :] + other).astype(out.dtype)

    def y_copy(slot):
        return remote(tx.at[slot], from_y.at[slot], y_send, y_recv.at[slot],
                      y_peer)

    sent, arrived = [], []

    def send(slots):
        for slot in slots:
            y_copy(slot).start()
            sent.append(slot)

    def receive(slots):
        for slot in slots:
            y_copy(slot).wait_recv()
            arrived.append(slot)

    def missing(block):
        return [s for s in range(_code_slot(block), _end_slot(block))
                if s not in arrived]

    encoder = _Encoder(tx)
    encoded = 0
    for load, n in zip(first_loads, FIRST_LOADS):
        load.wait()
        for block in range(encoded, encoded + n):
            nudged = block >= UNNUDGED_BLOCKS
            tiles = pairs(block, encoder.window.nudges if nudged else 0)
            send(encoder.put_bytes(block, tiles))
            if block == 0:
                encoder.place_window(tiles)
                first_tiles = tiles
                continue
            if block == 1:
                send(encoder.put_exponents(0, first_tiles))
            send(encoder.put_exponents(block, tiles))
        encoded += n

    @pl.when(mx == 0)
    def _():
        pl.semaphore_wait(x_ready, 1)

    head_load.wait()
    sum_copies = []
    for j, cols in enumerate(halves):
        at = (span(0, HEAD), cols)
        head_copies[j].wait_recv()
        out[at] = (own[at] + head[:, cols]).astype(out.dtype)
        sum_copies.append(
            remote(out.at[at], out.at[at], sum_send.at[j], sum_recv, x_peer))
        sum_copies[-1].start()

    y_load.wait()
    ready, held = [], []
    y_decoder, y_added = None, 0
    for i in range(X_SLOTS):
        slot = sent[i]
        receive([slot])
        part = next(p for p, (lo, hi) in enumerate(X_PARTS) if lo <= slot < hi)
        remote(from_y.at[slot], from_x.at[slot], x_send, x_recv.at[part],
               x_peer).start()
        if ready:
            send([ready.pop(0)])
        if encoded < Y_BLOCKS:
            tiles = pairs(encoded, encoder.window.nudges)
            held += encoder.put_bytes(encoded, tiles)
            codes = encoder.put_exponents(encoded, tiles)
            if codes:
                ready, held = ready + codes + held, []
            encoded += 1
        elif 0 not in sent:
            send(encoder.put_queue())
        if y_decoder is None and all(s in arrived for s in range(QUEUE_SLOTS)):
            y_decoder = _Decoder(from_y)
            for copy in (*head_copies, *sum_copies):
                copy.wait_send()
            wait_until_filled(out.at[span(M - HEAD, HEAD)], sum_recv)
        if y_decoder is not None and not missing(y_added):
            add(y_decoder, y_added, rows(y_added))
            y_added += 1
    send(ready)

    def receive_part(part):
        lo, hi = X_PARTS[part]
        wait_until_filled(from_x.at[lo:hi], x_recv.at[part])

    x_load.wait()
    receive_part(0)
    x_decoder = _Decoder(from_x)
    any_overflow = jnp.max(
        _overflowed(tx) | _overflowed(from_y) | _overflowed(from_x)) > 0
    while not missing(y_added):
        add(y_decoder, y_added, rows(y_added))
        y_added += 1
    for block in range(X_BLOCKS - 1):
        if block >= EARLY_X_BLOCKS:
            receive_part(block - EARLY_X_BLOCKS + 1)
        if X_BLOCKS - block <= Y_BLOCKS - y_added:
            receive(missing(y_added))
            add(y_decoder, y_added, rows(y_added))
            y_added += 1
        add(x_decoder, block, relayed_rows(block))

    assert y_added == Y_BLOCKS - 1
    last_y = y_decoder.exponents(Y_BLOCKS - 1)
    last_x = x_decoder.exponents(X_BLOCKS - 1)
    remote(from_y.at[:X_SLOTS], from_x, x_send, x_recv.at[0],
           x_peer).wait_send()
    remote(tx, from_y, y_send, y_recv.at[0], y_peer).wait_send()
    receive(missing(Y_BLOCKS - 1))
    add(y_decoder, Y_BLOCKS - 1, rows(Y_BLOCKS - 1), last_y)
    receive_part(len(X_PARTS) - 1)
    add(x_decoder, X_BLOCKS - 1, relayed_rows(X_BLOCKS - 1), last_x)
    assert sorted(sent) == sorted(arrived) == list(range(Y_SLOTS))

    @pl.when(any_overflow)
    def _():
        pieces = [pl.ds(2 * b, 2 * REDO_BLOCKS)
                  for b in range(0, Y_BLOCKS, REDO_BLOCKS)]
        y_copies = [
            remote(exp_tx.at[p], exp_from_y.at[p], exp_y_send.at[i],
                   exp_y_recv.at[i], y_peer)
            for i, p in enumerate(pieces)
        ]

        def redo(decoder, full, n_blocks, where):
            @pl.loop(0, n_blocks)
            def _(block):
                a, b = full[2 * block], full[2 * block + 1]
                shifted = (a << 7, srl(a, 1), b << 7, srl(b, 1))
                add(decoder, block, where(block),
                    [e & _both(0x7F80) for e in shifted])

        mine = jnp.max(_overflowed(tx)) > 0

        @pl.when(mine)
        def _():
            @pl.loop(0, Y_BLOCKS)
            def _(block):
                tiles = pairs(block, encoder.window.nudge(block))
                for k in range(2):
                    a, b = tiles[2 * k], tiles[2 * k + 1]
                    exp_tx[2 * block + k] = (
                        (srl(a, 7) & _both(0xFF)) | ((b << 1) & _both(0xFF00)))

            for copy in y_copies:
                copy.start()

        @pl.when(jnp.max(_overflowed(from_y)) > 0)
        def _():
            x_copies = [
                remote(exp_from_y.at[p], exp_from_x.at[p], exp_x_send.at[i],
                       exp_x_recv, x_peer)
                for i, p in enumerate(pieces[:X_BLOCKS // REDO_BLOCKS])
            ]
            for i, copy in enumerate(y_copies):
                copy.wait_recv()
                if i < len(x_copies):
                    x_copies[i].start()
            redo(y_decoder, exp_from_y, Y_BLOCKS, rows)
            for copy in x_copies:
                copy.wait_send()

        @pl.when(jnp.max(_overflowed(from_x)) > 0)
        def _():
            wait_until_filled(exp_from_x, exp_x_recv)
            redo(x_decoder, exp_from_x, X_BLOCKS, relayed_rows)

        @pl.when(mine)
        def _():
            for copy in y_copies:
                copy.wait_send()


def pallas_dist_ar_xy_y_m1024_n512_kernel(x: jax.Array):
    assert Y_BLOCKS % REDO_BLOCKS == 0 and X_BLOCKS % REDO_BLOCKS == 0
    dma = pltpu.SemaphoreType.DMA
    return pl.pallas_call(
        _body,
        out_shape=jax.ShapeDtypeStruct((M, N), jnp.bfloat16),
        in_specs=[pl.BlockSpec(memory_space=pl.ANY)],
        out_specs=pl.BlockSpec(memory_space=pltpu.VMEM),
        scratch_shapes=[
            pltpu.VMEM((M, N), jnp.float32),
            pltpu.VMEM((Y_SLOTS, *VREG), jnp.int32),
            pltpu.VMEM((Y_SLOTS, *VREG), jnp.int32),
            pltpu.VMEM((X_SLOTS, *VREG), jnp.int32),
            pltpu.VMEM((HEAD, N), jnp.float32),
            pltpu.VMEM((2 * Y_BLOCKS, *VREG), jnp.int32),
            pltpu.VMEM((2 * Y_BLOCKS, *VREG), jnp.int32),
            pltpu.VMEM((2 * X_BLOCKS, *VREG), jnp.int32),
            dma((len(FIRST_LOADS) + 3,)),
            dma((2,)),
            dma((2,)),
            dma,
            dma((Y_SLOTS,)),
            dma,
            dma((len(X_PARTS),)),
            dma((2,)),
            dma,
            dma((Y_BLOCKS // REDO_BLOCKS,)),
            dma((Y_BLOCKS // REDO_BLOCKS,)),
            dma((X_BLOCKS // REDO_BLOCKS,)),
            dma,
            pltpu.SemaphoreType.REGULAR,
        ],
        compiler_params=pltpu.CompilerParams(
            collective_id=0,
            disable_bounds_checks=True,
            disable_semaphore_checks=True,
        ),
    )(x)
```
